```python
import numpy as np

kernel_name = "dist_matmul_relu_kshard_i_m1024_n1024_k512"

def setup_inputs():
    A = np.random.randn(1024, 2048).astype(np.float32)
    B = np.random.randn(2048, 1024).astype(np.float32)
    return {"A": A, "B": B}

def reference(A: np.ndarray, B: np.ndarray) -> np.ndarray:
    z = A @ B
    return np.maximum(z, 0.0)
```

```python
import jax
import jax.numpy as jnp
from jax import lax
from jax.experimental import pallas as pl
from jax.experimental.pallas import tpu as pltpu

M, N, KS = 1024, 1024, 512
RB = 128

BF = jnp.bfloat16
F32 = jnp.float32


def make(ch_a=(256, 256, 512), ch_r=(512, 512), ch_f=(512, 384, 128), ch_o=(1024,)):
    def offs(ch):
        o, t = [], 0
        for c in ch:
            o.append((t, c))
            t += c
        assert t == N
        return o

    CA, CR, CF, CO = offs(ch_a), offs(ch_r), offs(ch_f), offs(ch_o)

    def body(a_hbm, b_hbm, o_hbm, a32, b32, a16, b16, acc, s1, r1, s2, r2, g,
             sem_a, sem_b, s1s, s1r, s2s, s2r, g1s, g1r, g2s, g2r, g3s, g3r):
        me = lax.axis_index("i")
        x = me // 2
        y = (me % 2) ^ x
        nbr = (me ^ 1, me ^ 3)
        u = (y, x)
        v = (x, y)
        bar = pltpu.get_barrier_semaphore()
        for p in nbr:
            pl.semaphore_signal(bar, inc=1, device_id=(p,), device_id_type=pl.DeviceIdType.MESH)

        def row(h, uu, vv):
            return pl.multiple_of((4 * h + 2 * uu + vv) * RB, RB)

        def arow(s, h):
            uu = 1 - u[h] if s < 2 else u[h]
            vv = 1 - v[h] if s % 2 == 0 else v[h]
            return row(h, uu, vv)

        a_cp = [[pltpu.make_async_copy(a_hbm.at[pl.ds(arow(s, h), RB)],
                                       a32.at[pl.ds((2 * s + h) * RB, RB)], sem_a.at[2 * s + h])
                 for h in range(2)] for s in range(4)]
        b_cp = [pltpu.make_async_copy(b_hbm.at[:, pl.ds(o, c)], b32.at[:, pl.ds(o, c)], sem_b.at[i])
                for i, (o, c) in enumerate(CA)]
        b_cp[0].start()
        a_cp[0][0].start()
        a_cp[0][1].start()
        for cp in b_cp[1:]:
            cp.start()
        for s in range(1, 4):
            for h in range(2):
                a_cp[s][h].start()

        def rcopy(src, dst, ss, rs, link):
            return pltpu.make_async_remote_copy(src, dst, ss, rs, device_id=(nbr[link],),
                                                device_id_type=pl.DeviceIdType.MESH)

        def cast_a(s):
            for h in range(2):
                a_cp[s][h].wait()
            rs = pl.ds(2 * s * RB, 2 * RB)
            a16[rs, :] = a32[rs, :].astype(BF)

        pend = []
        rs1 = [[], []]
        for i, (o, c) in enumerate(CA):
            cs = pl.ds(o, c)
            b_cp[i].wait()
            b16[:, cs] = b32[:, cs].astype(BF)
            if i == 0:
                cast_a(0)
            z = jnp.dot(a16[pl.ds(0, 2 * RB), :], b16[:, cs], preferred_element_type=F32)
            s1[pl.ds(0, 2 * RB), cs] = z.astype(BF)
            if i == 0:
                pl.semaphore_wait(bar, 2)
            for h in range(2):
                rs = pl.ds(h * RB, RB)
                cp = rcopy(s1.at[rs, cs], r1.at[rs, cs], s1s.at[2 * i + h], s1r.at[2 * i + h], h)
                cp.start()
                rs1[h].append(cp)
        cast_a(1)
        z = jnp.dot(a16[pl.ds(2 * RB, 2 * RB), :], b16[...], preferred_element_type=F32)
        s1[pl.ds(2 * RB, 2 * RB), :] = z.astype(BF)
        rs1b = []
        for h in range(2):
            rs = pl.ds((2 + h) * RB, RB)
            k = 2 * len(CA) + h
            cp = rcopy(s1.at[rs], r1.at[rs], s1s.at[k], s1r.at[k], h)
            cp.start()
            rs1b.append(cp)
        cast_a(2)
        acc[pl.ds(0, 2 * RB), :] = jnp.dot(a16[pl.ds(4 * RB, 2 * RB), :], b16[...], preferred_element_type=F32)
        cast_a(3)
        acc[pl.ds(2 * RB, 2 * RB), :] = jnp.dot(a16[pl.ds(6 * RB, 2 * RB), :], b16[...], preferred_element_type=F32)
        for h in range(2):
            for cp in rs1[h]:
                cp.wait_recv()
        rs2 = [[], []]
        for i, (o, c) in enumerate(CR):
            cs = pl.ds(o, c)
            rs = pl.ds(0, 2 * RB)
            s2[rs, cs] = (acc[rs, cs] + r1[rs, cs].astype(F32)).astype(BF)
            for h in range(2):
                rs = pl.ds(h * RB, RB)
                cp = rcopy(s2.at[rs, cs], r2.at[rs, cs], s2s.at[2 * i + h], s2r.at[2 * i + h], 1 - h)
                cp.start()
                rs2[h].append(cp)
        for h in range(2):
            rs1b[h].wait_recv()
        ocp = []

        def emit(k, h, ci, o, c):
            cs = pl.ds(o, c)
            rs = pl.ds((2 * k + h) * RB, RB)
            o_hbm[pl.ds(arow(3 - k, h), RB), cs] = g[rs, cs].astype(F32)

        ag1 = [[], []]
        for i, (o, c) in enumerate(CR):
            cs = pl.ds(o, c)
            for h in range(2):
                rs2[h][i].wait_recv()
            lo, hi = pl.ds(0, 2 * RB), pl.ds(2 * RB, 2 * RB)
            z = acc[hi, cs] + r1[hi, cs].astype(F32) + r2[lo, cs].astype(F32)
            g[lo, cs] = jnp.maximum(z, 0.0).astype(BF)
            for h in range(2):
                cp = rcopy(g.at[pl.ds(h * RB, RB), cs], g.at[pl.ds((2 + h) * RB, RB), cs],
                           g1s.at[2 * i + h], g1r.at[2 * i + h], 1 - h)
                cp.start()
                ag1[h].append(cp)
            for h in range(2):
                emit(0, h, i, o, c)
        ag2 = [[], []]
        for i, (o, c) in enumerate(CO):
            cs = pl.ds(o, c)
            for h in range(2):
                cp = rcopy(g.at[pl.ds(h * RB, RB), cs], g.at[pl.ds((4 + h) * RB, RB), cs],
                           g2s.at[2 * i + h], g2r.at[2 * i + h], h)
                cp.start()
                ag2[h].append(cp)
        for i, (o, c) in enumerate(CR):
            for h in range(2):
                ag1[h][i].wait_recv()
            if i < len(CR) - 1:
                for h in range(2):
                    emit(1, h, i, o, c)
        ag3 = [[], []]
        for i, (o, c) in enumerate(CF):
            cs = pl.ds(o, c)
            for h in range(2):
                cp = rcopy(g.at[pl.ds((2 + h) * RB, RB), cs], g.at[pl.ds((6 + h) * RB, RB), cs],
                           g3s.at[2 * i + h], g3r.at[2 * i + h], h)
                cp.start()
                ag3[h].append(cp)
        for h in range(2):
            emit(1, h, len(CR) - 1, *CR[-1])
        for lst in (rs1, [[c] for c in rs1b], rs2, ag1):
            for h in range(2):
                for cp in lst[h]:
                    cp.wait_send()
        for i, (o, c) in enumerate(CO):
            for h in range(2):
                ag2[h][i].wait_recv()
                emit(2, h, i, o, c)
        for i, (o, c) in enumerate(CF):
            for h in range(2):
                ag3[h][i].wait_recv()
                emit(3, h, i, o, c)
        for lst in (ag2, ag3):
            for h in range(2):
                for cp in lst[h]:
                    cp.wait_send()
        for cp in ocp:
            cp.wait()

    n_o = 2 * (2 * len(CR) + len(CO) + len(CF))
    DMA = pltpu.SemaphoreType.DMA

    def fn(A, B):
        return pl.pallas_call(
            body,
            out_shape=jax.ShapeDtypeStruct((M, N), F32),
            in_specs=[pl.BlockSpec(memory_space=pltpu.HBM)] * 2,
            out_specs=pl.BlockSpec(memory_space=pltpu.VMEM),
            scratch_shapes=[
                pltpu.VMEM((M, KS), F32), pltpu.VMEM((KS, N), F32),
                pltpu.VMEM((M, KS), BF), pltpu.VMEM((KS, N), BF),
                pltpu.VMEM((4 * RB, N), F32),
                pltpu.VMEM((4 * RB, N), BF), pltpu.VMEM((4 * RB, N), BF),
                pltpu.VMEM((2 * RB, N), BF), pltpu.VMEM((2 * RB, N), BF),
                pltpu.VMEM((8 * RB, N), BF),
                DMA((8,)), DMA((len(CA),)),
                DMA((2 * len(CA) + 2,)), DMA((2 * len(CA) + 2,)),
                DMA((2 * len(CR),)), DMA((2 * len(CR),)),
                DMA((2 * len(CR),)), DMA((2 * len(CR),)),
                DMA((2 * len(CO),)), DMA((2 * len(CO),)),
                DMA((2 * len(CF),)), DMA((2 * len(CF),)),
            ],
            compiler_params=pltpu.CompilerParams(collective_id=0, vmem_limit_bytes=48 * 1024 * 1024),
        )(A, B)

    return fn


_kernel = make()


def pallas_dist_matmul_relu_kshard_i_m1024_n1024_k512_kernel(A: jax.Array, B: jax.Array):
    return _kernel(A, B)
```

```python
import contextlib
import jax
import jax.numpy as jnp
from jax import lax
from jax.experimental import pallas as pl
from jax.experimental.pallas import tpu as pltpu

M, N, KS = 1024, 1024, 512
RB = 128
L = 128
U = 256

BF = jnp.bfloat16
F32 = jnp.float32
I32 = jnp.int32
SIGN = -(1 << 31)


def i32(v):
    return v - (1 << 32) if v >= (1 << 31) else v


def rep(v):
    return i32(v | (v << 16))


def shl(x, n):
    return x if n == 0 else (lax.shift_left(x, n) if n > 0 else lax.shift_right_logical(x, -n))


def words(xv, signed):
    bits = pltpu.bitcast(xv, I32)
    mag = bits & 0x7FFFFFFF if signed else bits
    mx = pltpu.bitcast(jnp.max(pltpu.bitcast(mag, F32), axis=0, keepdims=True), I32)
    mn = pltpu.bitcast(jnp.max(pltpu.bitcast(SIGN - mag, F32), axis=0, keepdims=True), I32) & 0x7FFFFFFF
    k = jnp.maximum(lax.shift_right_logical(mx + 0x8000, 23) - 31, 0)
    miss = (k > 126) | (mn > SIGN - lax.shift_left(k + 1, 23))
    xv = xv * pltpu.bitcast(lax.shift_left(127 - k, 23), F32)
    w = pltpu.bitcast(pltpu.pack_elementwise([xv[:64], xv[64:]], packed_dtype=BF), I32)
    return jnp.where(miss, 0x80, k), w


def values(w, hdr):
    lo = pltpu.bitcast(lax.shift_left(w, 16), F32)
    hi = pltpu.bitcast(w & i32(0xFFFF0000), F32)
    return jnp.concatenate([lo, hi], axis=0) * pltpu.bitcast(lax.shift_left((hdr & 0x7F) + 127, 23), F32)


def squeeze12(w):
    e = w[48:64]
    return jnp.concatenate([w[16 * j:16 * j + 16] | (shl(e, 12 - 4 * j) & rep(0xF000)) for j in range(3)], axis=0)


def expand12(r):
    p = [r[16 * j:16 * j + 16] for j in range(3)]
    e = [shl(p[j] & rep(0xF000), 4 * j - 12) for j in range(3)]
    return jnp.concatenate([r & rep(0x0FFF), e[0] | e[1] | e[2]], axis=0)


def squeeze13(w):
    p = [w[8 * j:8 * j + 8] for j in range(16)]
    out = [p[j] | (shl(p[13 + j // 4], 12 - 3 * (j % 4)) & rep(0x7000)) for j in range(12)]
    s = [shl(p[13 + j] & rep(0x8000), -1 - j) for j in range(3)]
    out.append(p[12] | s[0] | s[1] | s[2])
    return jnp.concatenate(out, axis=0)


def expand13(r):
    p = [r[8 * j:8 * j + 8] for j in range(13)]
    ext = []
    for e in range(3):
        v = shl(p[12], 1 + e) & rep(0x8000)
        for q in range(4):
            v = v | shl(p[4 * e + q] & rep(0x7000), 3 * q - 12)
        ext.append(v)
    return jnp.concatenate([r & rep(0x8FFF)] + ext, axis=0)


def make(ramp=((0, 64, 0, 128), (64, 64, 0, 128), (0, 128, 128, 128)), relay=True, prio=None,
         nf=6, scopes=False, nochk=True, **cp_kw):
    def ns(name):
        return jax.named_scope(name) if scopes else contextlib.nullcontext()

    loads, need, have_r, have_c = [], [], 0, 0
    for r0, nr, c0, nc in ramp:
        if c0 + nc > have_c:
            loads.append(("b", have_c, c0 + nc - have_c))
            have_c = c0 + nc
        if r0 + nr > have_r:
            loads += [("a", 0, q, have_r, r0 + nr - have_r) for q in range(2)]
            have_r = r0 + nr
        need.append(len(loads))
    nl = len(loads)
    loads += [("a", 1, 0, 0, RB), ("a", 1, 1, 0, RB), ("b", U, U), ("b", 2 * U, 2 * U)]
    loads += [("a", s, q, 0, RB) for s in (2, 3) for q in range(2)]

    AT = {(1, 0): (0, 104, 0), (0, 1): (112, 216, 0), (1, 1): (224, 223, 0),
          (0, 3): (336, 335, 0), (0, 2): (440, 648, 0), (1, 2): (544, 648, 16), (1, 3): (656, 655, 0)}
    P1 = 760
    M10, M01, M11 = pl.ds(0, 105), pl.ds(112, 105), pl.ds(223, 105)
    MA, MX, MY, MB = pl.ds(335, 314), pl.ds(335, 105), pl.ds(440, 209), pl.ds(655, 105)
    P2 = 4 * 104 + 8
    M2 = (pl.ds(0, 209), pl.ds(215, 209))

    def at2(c):
        return 104 * c + 8 * (c // 2), 208 + 7 * (c // 2), 16 * (c % 2)

    PG = 8 * 48 + 8
    HG = 4 * 48
    AG1 = (pl.ds(0, HG + 1), pl.ds(HG + 7, HG + 1))

    def gro(j):
        return 48 * j + 8 * (j // 4)

    def ghdr(j):
        return HG + 7 * (j // 4)

    n_msg = len(ramp) + 4 + 4 + 1 + 2

    def body(a_hbm, b_hbm, o_ref, a32, b32, a16, b16, acc, s1, r1, ps1, pr1, ps2, pr2, pg, zb, px,
             fs1, fr1, fs2, fr2, fg, sem_in, sem_s, sem_r, sem_x, sem_fs, sem_fr):
        me = lax.axis_index("i")
        x = me >> 1
        y = (me & 1) ^ x
        first = jnp.where(me == 1, 1, 0)
        H = (first, 1 - first)

        def peer(link):
            return (me ^ (1 + 2 * link),)

        def grow(s, h, r0=0):
            uu = jnp.where(h == 0, y, x) ^ (1 - s // 2)
            vv = jnp.where(h == 0, x, y) ^ (1 - s % 2)
            return pl.multiple_of((4 * h + 2 * uu + vv) * RB + r0, 16)

        lcp = []
        for i, l in enumerate(loads):
            if l[0] == "a":
                _, s, q, r0, nr = l
                cp = pltpu.make_async_copy(a_hbm.at[pl.ds(grow(s, H[q], r0), nr)],
                                           a32.at[pl.ds((2 * s + q) * RB + r0, nr)], sem_in.at[i])
            else:
                _, c0, nc = l
                cp = pltpu.make_async_copy(b_hbm.at[:, pl.ds(c0, nc)], b32.at[:, pl.ds(c0, nc)], sem_in.at[i])
            cp.start(priority=prio(i, l) if prio else 0)
            lcp.append(cp)
            if i == 2:
                bar = pltpu.get_barrier_semaphore()
                for link in range(2):
                    pl.semaphore_signal(bar, inc=1, device_id=peer(link), device_id_type=pl.DeviceIdType.MESH)

        done = [0]

        def land(n):
            while done[0] < n:
                i = done[0]
                with ns(f"ld{i}"):
                    lcp[i].wait()
                l = loads[i]
                if l[0] == "a":
                    _, s, q, r0, nr = l
                    rs = pl.ds((2 * s + q) * RB + r0, nr)
                    a16[rs, :] = a32[rs, :].astype(BF)
                else:
                    _, c0, nc = l
                    b16[:, pl.ds(c0, nc)] = b32[:, pl.ds(c0, nc)].astype(BF)
                done[0] += 1

        def remote(src, dst, ssem, rsem, link):
            return pltpu.make_async_remote_copy(src, dst, ssem, rsem, device_id=peer(link),
                                                device_id_type=pl.DeviceIdType.MESH)

        sends = []

        def send(src, dst, h, link):
            cp = remote(src, dst, sem_s.at[link], sem_r.at[len(sends) // 2 * 2 + h], link)
            cp.start()
            sends.append(cp)
            return cp

        def mm(blocks, c0, nc, r0=0, nr=RB):
            lhs = jnp.concatenate([a16[pl.ds(b * RB + r0, nr), :] for b in blocks], axis=0)
            return jnp.dot(lhs, b16[:, pl.ds(c0, nc)], preferred_element_type=F32)

        def put_unit(buf, h, at, xv, flags=0):
            row, hrow, bit = at
            (h0, w0), (h1, w1) = words(xv[:, :L], True), words(xv[:, L:], True)
            hd = shl(h0 | shl(h1, 8) | flags, bit)
            buf[h, pl.ds(hrow, 1), :] = hd | buf[h, pl.ds(hrow, 1), :] if bit else hd
            buf[h, pl.ds(row, 104), :] = squeeze13(jnp.concatenate([w0, w1], axis=0))

        def get_unit(buf, h, at, live=None):
            row, hrow, bit = at
            w = expand13(buf[h, pl.ds(row, 104), :])
            hd = shl(buf[h, pl.ds(hrow, 1), :], -bit)
            vals = [values(w[:64], hd), values(w[64:], shl(hd, -8))]
            flags = hd & 0x8080
            if live is not None:
                vals = [jnp.where(live, t, 0.0) for t in vals]
                flags = jnp.where(live, flags, 0)
            return vals, flags

        ramp_cp = [[], []]
        for i, (r0, nr, c0, nc) in enumerate(ramp):
            land(need[i])
            z = mm((0, 1), c0, nc, r0, nr).astype(BF)
            for q, h in enumerate(H):
                s1[h, pl.ds(r0, nr), pl.ds(c0, nc)] = z[q * nr:(q + 1) * nr]
            if i == 0:
                with ns("bar"):
                    pl.semaphore_wait(bar, 2)
            for q, h in enumerate(H):
                ramp_cp[q].append(send(s1.at[h, pl.ds(r0, nr), pl.ds(c0, nc)],
                                       r1.at[h, pl.ds(r0, nr), pl.ds(c0, nc)], h, h))
        c10, c01, c11, c13 = [], [], [], []
        for q, h in enumerate(H):
            land(nl + 1 + q)
            put_unit(ps1, h, AT[1, 0], mm((2 + q,), 0, U))
            c10.append(send(ps1.at[h, M10], pr1.at[h, M10], h, h))
        land(nl + 3)
        for s, lst, ms in ((0, c01, M01), (1, c11, M11)):
            z = mm((2 * s, 2 * s + 1), U, U)
            for q, h in enumerate(H):
                put_unit(ps1, h, AT[s, 1], z[q * RB:(q + 1) * RB])
                lst.append(send(ps1.at[h, ms], pr1.at[h, ms], h, h))

        via2 = [(me == 1 + 2 * h) if relay else (me < 0) for h in H]
        is0, is2 = ((me == 0), (me == 2)) if relay else (me < 0, me < 0)

        def cp_a(h, ms):
            return remote(ps1.at[h, ms], pr1.at[h, ms], sem_x.at[h], sem_x.at[2 + h], h)

        def cp_x(h):
            return remote(ps1.at[h, MX], px.at[h, pl.ds(7, 105)], sem_x.at[4], sem_x.at[5 + h], 1 - h)

        land(nl + 4)
        z = mm((0, 1), 2 * U, 2 * U)
        for q, h in enumerate(H):
            for c in (3, 2):
                put_unit(ps1, h, AT[0, c], z[q * RB:(q + 1) * RB, (c - 2) * U:(c - 1) * U])
        for q, h in enumerate(H):
            pl.when(via2[q])(lambda: cp_x(h).start())
        z = mm((2, 3), 2 * U, 2 * U)
        zb[...] = z[:, U:]
        for q, h in enumerate(H):
            put_unit(ps1, h, AT[1, 2], z[q * RB:(q + 1) * RB, :U])
        for q, h in enumerate(H):
            pl.when(via2[q])(lambda: cp_a(h, MY).start())
            pl.when(jnp.logical_not(via2[q]))(lambda: cp_a(h, MA).start())

        land(nl + 6)
        acc[pl.ds(0, 2 * RB), :] = mm((4, 5), 0, N)
        with ns("px"):
            @pl.when(is2)
            def _():
                for h in range(2):
                    cp_x(h).wait_recv()
        for q, h in enumerate(H):
            p, flags = get_unit(px, h, (8, 7, 0), is2)
            put_unit(ps1, h, AT[1, 3], zb[pl.ds(q * RB, RB), :] + jnp.concatenate(p, axis=1), flags)
            c13.append(send(ps1.at[h, MB], pr1.at[h, MB], h, h))
        land(nl + 8)
        acc[pl.ds(2 * RB, 2 * RB), :] = mm((6, 7), 0, N)
        got = set()

        def partner(s, c, q):
            h = H[q]
            msg = {(0, 0): ramp_cp[q], (1, 0): [c10[q]], (0, 1): [c01[q]], (1, 1): [c11[q]],
                   (1, 3): [c13[q]]}.get((s, c))
            key = (q, id(msg[0]) if msg else None)
            if key not in got:
                got.add(key)
                with ns(f"rs1_{s}{c}_{q}"):
                    for cp in msg or ():
                        cp.wait_recv()
                    if not msg:
                        pl.when(is0)(lambda: cp_a(h, MY).wait_recv())
                        pl.when(jnp.logical_not(is0))(lambda: cp_a(h, MA).wait_recv())
            if (s, c) == (0, 0):
                return [r1[h, :, pl.ds(e * L, L)].astype(F32) for e in range(2)], 0
            return get_unit(pr1, h, AT[s, c], jnp.logical_not(is0) if (s, c) == (0, 3) else None)

        rs2 = [[], []]
        for i in range(2):
            for q, h in enumerate(H):
                for c in (2 * i, 2 * i + 1):
                    p, flags = partner(0, c, q)
                    put_unit(ps2, h, at2(c), acc[pl.ds(q * RB, RB), pl.ds(c * U, U)] + jnp.concatenate(p, axis=1),
                             flags)
                rs2[q].append(send(ps2.at[h, M2[i]], pr2.at[h, M2[i]], h, 1 - h))

        ag1 = [[], []]
        for i in range(2):
            for q, h in enumerate(H):
                with ns(f"rs2_{i}_{q}"):
                    rs2[q][i].wait_recv()
                hdr = 0
                for c in (2 * i, 2 * i + 1):
                    p1, f1 = partner(1, c, q)
                    p2, f2 = get_unit(pr2, h, at2(c))
                    hdr = hdr | shl(f1 | f2, 16 * (c % 2))
                    for e in range(2):
                        j = 2 * c + e
                        xv = jnp.maximum(acc[pl.ds((2 + q) * RB, RB), pl.ds(j * L, L)] + p1[e] + p2[e], 0.0)
                        hd, w = words(xv, False)
                        hdr = hdr | shl(hd, 8 * (j % 4))
                        pg[h, pl.ds(gro(j), 48), :] = squeeze12(w)
                pg[h, pl.ds(ghdr(4 * i), 1), :] = hdr
                ag1[q].append(send(pg.at[h, AG1[i]], pg.at[2 + h, AG1[i]], h, 1 - h))
        ag2 = [send(pg.at[h], pg.at[4 + h], h, h) for h in H]

        def emit(k, h, js):
            for j in js:
                o_ref[pl.ds(grow(3 - k, h), RB), pl.ds(j * L, L)] = values(
                    expand12(pg[2 * k + h, pl.ds(gro(j), 48), :]),
                    shl(pg[2 * k + h, pl.ds(ghdr(j), 1), :], -8 * (j % 4)))

        for h in H:
            emit(0, h, range(8))
        AG3 = (pl.ds(0, gro(nf)), pl.ds(gro(nf), PG - gro(nf)))
        ag3 = []
        for q, h in enumerate(H):
            with ns(f"ag1_{q}"):
                for cp in ag1[q]:
                    cp.wait_recv()
            ag3.append([remote(pg.at[2 + h, ms], pg.at[6 + h, ms], sem_s.at[h], sem_r.at[2 * (n_msg - 2 + e) + h], h)
                        for e, ms in enumerate(AG3)])
            for cp in ag3[q]:
                cp.start()
        for h in H:
            emit(1, h, range(8))
        for q in (1, 0):
            with ns(f"ag2_{q}"):
                ag2[q].wait_recv()
            emit(2, H[q], range(8))
        for q in (1, 0):
            with ns(f"ag3a_{q}"):
                ag3[q][0].wait_recv()
            emit(3, H[q], range(nf))
        flags = 0
        for k in range(8):
            flags = flags | pg[k, pl.ds(ghdr(0), 1), :] | pg[k, pl.ds(ghdr(4), 1), :]
        miss = jnp.max(shl(flags & i32(0x80808080), -1)) > 0
        with ns("snd"):
            for cp in sends + ag3[0] + ag3[1]:
                cp.wait_send()
            for q, h in enumerate(H):
                @pl.when(via2[q])
                def _():
                    cp_x(h).wait_send()
                    cp_a(h, MY).wait_send()
                pl.when(jnp.logical_not(via2[q]))(lambda: cp_a(h, MA).wait_send())

        @pl.when(miss)
        def _():
            for q in range(2):
                ag3[q][1].wait_recv()

            def exchange(k, src, dst, first_link):
                cps = [remote(src(h), dst(h), sem_fs.at[h], sem_fr.at[2 * k + h], h if first_link else 1 - h)
                       for h in range(2)]
                for cp in cps:
                    cp.start()
                for cp in cps:
                    cp.wait()

            def tiles(n, f):
                @pl.loop(0, n * 4)
                def _(t):
                    f(t >> 2, pl.ds(pl.multiple_of((t & 3) * U, U), U))

            def rows(i):
                return pl.ds(pl.multiple_of(i * RB, RB), RB)

            def f1(i, cs):
                z = jnp.dot(a16[rows(2 * (i & 1) + ((i >> 1) ^ first)), :], b16[:, cs], preferred_element_type=F32)
                fs1[rows(i), cs] = z.astype(BF)
            tiles(4, f1)
            exchange(0, lambda h: fs1.at[pl.ds(2 * h * RB, 2 * RB)], lambda h: fr1.at[pl.ds(2 * h * RB, 2 * RB)], True)

            def f2(h, cs):
                fs2[rows(h), cs] = (acc[rows(h ^ first), cs] + fr1[rows(2 * h), cs].astype(F32)).astype(BF)
            tiles(2, f2)
            exchange(1, lambda h: fs2.at[pl.ds(h * RB, RB)], lambda h: fr2.at[pl.ds(h * RB, RB)], False)

            def f3(h, cs):
                z = (acc[rows(2 + (h ^ first)), cs] + fr1[rows(2 * h + 1), cs].astype(F32)
                     + fr2[rows(h), cs].astype(F32))
                fg[rows(4 * h), cs] = jnp.maximum(z, 0.0).astype(BF)
            tiles(2, f3)
            exchange(2, lambda h: fg.at[pl.ds(4 * h * RB, RB)], lambda h: fg.at[pl.ds((4 * h + 1) * RB, RB)], False)
            exchange(3, lambda h: fg.at[pl.ds(4 * h * RB, 2 * RB)], lambda h: fg.at[pl.ds((4 * h + 2) * RB, 2 * RB)],
                     True)

            def f4(i, cs):
                h = i >> 2
                uu = jnp.where(h == 0, y, x) ^ ((i >> 1) & 1)
                vv = jnp.where(h == 0, x, y) ^ (i & 1)
                o_ref[rows(4 * h + 2 * uu + vv), cs] = fg[rows(i), cs].astype(F32)
            tiles(8, f4)

        @pl.when(jnp.logical_not(miss))
        def _():
            for q in (1, 0):
                with ns(f"ag3b_{q}"):
                    ag3[q][1].wait_recv()
                emit(3, H[q], range(nf, 8))

    DMA = pltpu.SemaphoreType.DMA

    def fn(A, B):
        return pl.pallas_call(
            body,
            out_shape=jax.ShapeDtypeStruct((M, N), F32),
            in_specs=[pl.BlockSpec(memory_space=pltpu.HBM)] * 2,
            out_specs=pl.BlockSpec(memory_space=pltpu.VMEM),
            scratch_shapes=[
                pltpu.VMEM((M, KS), F32), pltpu.VMEM((KS, N), F32),
                pltpu.VMEM((M, KS), BF), pltpu.VMEM((KS, N), BF),
                pltpu.VMEM((4 * RB, N), F32),
                pltpu.VMEM((2, RB, U), BF), pltpu.VMEM((2, RB, U), BF),
                pltpu.VMEM((2, P1, L), I32), pltpu.VMEM((2, P1, L), I32),
                pltpu.VMEM((2, P2, L), I32), pltpu.VMEM((2, P2, L), I32),
                pltpu.VMEM((8, PG, L), I32),
                pltpu.VMEM((2 * RB, U), F32), pltpu.VMEM((2, 112, L), I32),
                pltpu.VMEM((4 * RB, N), BF), pltpu.VMEM((4 * RB, N), BF),
                pltpu.VMEM((2 * RB, N), BF), pltpu.VMEM((2 * RB, N), BF),
                pltpu.VMEM((8 * RB, N), BF),
                DMA((len(loads),)), DMA((2,)), DMA((2 * n_msg,)), DMA((7,)), DMA((2,)), DMA((8,)),
            ],
            compiler_params=pltpu.CompilerParams(collective_id=0, vmem_limit_bytes=48 * 1024 * 1024,
                                                 disable_bounds_checks=nochk, disable_semaphore_checks=nochk,
                                                 **cp_kw),
        )(A, B)

    return fn


_kernel = make()


def pallas_dist_matmul_relu_kshard_i_m1024_n1024_k512_kernel(A: jax.Array, B: jax.Array):
    return _kernel(A, B)
```

```python
import jax
import jax.numpy as jnp
from jax import lax
from jax.experimental import pallas as pl
from jax.experimental.pallas import tpu as pltpu

M, N, KS = 1024, 1024, 512
RB = 128
L = 128
U = 256

BF, F32, I32 = jnp.bfloat16, jnp.float32, jnp.int32
SIGN = -(1 << 31)


def _i32(v):
    return v - (1 << 32) if v >= (1 << 31) else v


def _rep(v):
    return _i32(v | (v << 16))


def _shl(x, n):
    return x if n == 0 else (lax.shift_left(x, n) if n > 0 else lax.shift_right_logical(x, -n))


def _words(tile, signed):
    bits = pltpu.bitcast(tile, I32)
    mag = bits & 0x7FFFFFFF if signed else bits
    top = pltpu.bitcast(jnp.max(pltpu.bitcast(mag, F32), axis=0, keepdims=True), I32)
    low = pltpu.bitcast(jnp.max(pltpu.bitcast(SIGN - mag, F32), axis=0, keepdims=True), I32) & 0x7FFFFFFF
    base = jnp.maximum(lax.shift_right_logical(top + 0x8000, 23) - 31, 0)
    miss = (base > 126) | (low > SIGN - lax.shift_left(base + 1, 23))
    tile = tile * pltpu.bitcast(lax.shift_left(127 - base, 23), F32)
    w = pltpu.bitcast(pltpu.pack_elementwise([tile[:64], tile[64:]], packed_dtype=BF), I32)
    return jnp.where(miss, 0x80, base), w


def _values(w, hdr):
    lo = pltpu.bitcast(lax.shift_left(w, 16), F32)
    hi = pltpu.bitcast(w & _i32(0xFFFF0000), F32)
    return jnp.concatenate([lo, hi], axis=0) * pltpu.bitcast(lax.shift_left((hdr & 0x7F) + 127, 23), F32)


def _squeeze12(w):
    return jnp.concatenate([w[16 * j:16 * j + 16] | (_shl(w[48:], 12 - 4 * j) & _rep(0xF000)) for j in range(3)],
                           axis=0)


def _expand12(r):
    e = [_shl(r[16 * j:16 * j + 16] & _rep(0xF000), 4 * j - 12) for j in range(3)]
    return jnp.concatenate([r & _rep(0x0FFF), e[0] | e[1] | e[2]], axis=0)


def _squeeze13(w):
    p = [w[8 * j:8 * j + 8] for j in range(16)]
    out = [p[j] | (_shl(p[13 + j // 4], 12 - 3 * (j % 4)) & _rep(0x7000)) for j in range(12)]
    s = [_shl(p[13 + j] & _rep(0x8000), -1 - j) for j in range(3)]
    return jnp.concatenate(out + [p[12] | s[0] | s[1] | s[2]], axis=0)


def _expand13(r):
    p = [r[8 * j:8 * j + 8] for j in range(13)]
    ext = []
    for e in range(3):
        v = _shl(p[12], 1 + e) & _rep(0x8000)
        for q in range(4):
            v = v | _shl(p[4 * e + q] & _rep(0x7000), 3 * q - 12)
        ext.append(v)
    return jnp.concatenate([r & _rep(0x8FFF)] + ext, axis=0)


RAMP = ((0, 64, 0), (64, 64, 0), (0, 128, L))
LOADS = (
    ("b", 0, L), ("a", 0, 0, 0, 64), ("a", 0, 1, 0, 64), ("a", 0, 0, 64, 64), ("a", 0, 1, 64, 64), ("b", L, L),
    ("a", 1, 0, 0, RB), ("a", 1, 1, 0, RB), ("b", U, U), ("b", 2 * U, 2 * U),
    ("a", 2, 0, 0, RB), ("a", 2, 1, 0, RB), ("a", 3, 0, 0, RB), ("a", 3, 1, 0, RB),
)
RAMP_NEEDS = (3, 5, 6)

AT1 = {(1, 0): (0, 104, 0), (0, 1): (112, 216, 0), (1, 1): (224, 223, 0),
       (0, 3): (336, 335, 0), (0, 2): (440, 648, 0), (1, 2): (544, 648, 16), (1, 3): (656, 655, 0)}
P1 = 760
M10, M01, M11, M13 = (0, 105), (112, 105), (223, 105), (655, 105)
MA, MX, MY = (335, 314), (335, 105), (440, 209)
AT2 = tuple((104 * c + 8 * (c // 2), 208 + 7 * (c // 2), 16 * (c % 2)) for c in range(4))
P2 = 424
M2 = ((0, 209), (215, 209))
G_ROW = tuple(48 * j + 2 * (j // 4) for j in range(8))
G_HDR = tuple(192 + j // 4 for j in range(8))
PG = 386
AG_OWN = ((0, 193), (193, 193))
NF = 6
AG_FWD = ((0, G_ROW[NF]), (G_ROW[NF], PG - G_ROW[NF]))
N_MSG = len(RAMP) + 4 + 2 + 2 + 1 + 2


def _body(a_hbm, b_hbm, o_ref, a32, b32, a16, b16, acc, s1, r1, ps1, pr1, ps2, pr2, pg, zb, px,
          fs1, fr1, fs2, fr2, fg, sem_in, sem_s, sem_r, sem_x, sem_fs, sem_fr):
    me = lax.axis_index("i")
    x = me >> 1
    y = (me & 1) ^ x
    first = jnp.where(me == 1, 1, 0)
    H = (first, 1 - first)
    is0, is2 = me == 0, me == 2

    def peer(link):
        return (me ^ (1 + 2 * link),)

    def block_row(s, h, r0=0):
        u = jnp.where(h == 0, y, x) ^ (1 - s // 2)
        v = jnp.where(h == 0, x, y) ^ (1 - s % 2)
        return pl.multiple_of((4 * h + 2 * u + v) * RB + r0, 16)

    loads = []
    for i, ld in enumerate(LOADS):
        if ld[0] == "a":
            _, s, q, r0, nr = ld
            cp = pltpu.make_async_copy(a_hbm.at[pl.ds(block_row(s, H[q], r0), nr)],
                                       a32.at[pl.ds((2 * s + q) * RB + r0, nr)], sem_in.at[i])
        else:
            cs = pl.ds(*ld[1:])
            cp = pltpu.make_async_copy(b_hbm.at[:, cs], b32.at[:, cs], sem_in.at[i])
        cp.start()
        loads.append(cp)
        if i == RAMP_NEEDS[0] - 1:
            barrier = pltpu.get_barrier_semaphore()
            for link in range(2):
                pl.semaphore_signal(barrier, inc=1, device_id=peer(link), device_id_type=pl.DeviceIdType.MESH)
    landed = [0]

    def land(n):
        for i in range(landed[0], n):
            loads[i].wait()
            if LOADS[i][0] == "a":
                _, s, q, r0, nr = LOADS[i]
                rs = pl.ds((2 * s + q) * RB + r0, nr)
                a16[rs, :] = a32[rs, :].astype(BF)
            else:
                cs = pl.ds(*LOADS[i][1:])
                b16[:, cs] = b32[:, cs].astype(BF)
        landed[0] = n

    def remote(src, dst, send_sem, recv_sem, link):
        return pltpu.make_async_remote_copy(src, dst, send_sem, recv_sem, device_id=peer(link),
                                            device_id_type=pl.DeviceIdType.MESH)

    sent = []

    def send(src, dst, h, link):
        k = len(sent) // 2 * 2 + h
        cp = remote(src, dst, sem_s.at[k], sem_r.at[k], link)
        cp.start()
        sent.append(cp)
        return cp

    def send1(h, msg):
        return send(ps1.at[h, pl.ds(*msg)], pr1.at[h, pl.ds(*msg)], h, h)

    def mm(blocks, c0, nc, r0=0, nr=RB):
        lhs = jnp.concatenate([a16[pl.ds(b * RB + r0, nr), :] for b in blocks], axis=0)
        return jnp.dot(lhs, b16[:, pl.ds(c0, nc)], preferred_element_type=F32)

    def put_unit(buf, h, at, vals, flags=0):
        row, hrow, bit = at
        (h0, w0), (h1, w1) = _words(vals[:, :L], True), _words(vals[:, L:], True)
        hdr = _shl(h0 | _shl(h1, 8) | flags, bit)
        buf[h, pl.ds(hrow, 1), :] = hdr | buf[h, pl.ds(hrow, 1), :] if bit else hdr
        buf[h, pl.ds(row, 104), :] = _squeeze13(jnp.concatenate([w0, w1], axis=0))

    def get_unit(buf, h, at, live=None):
        row, hrow, bit = at
        w = _expand13(buf[h, pl.ds(row, 104), :])
        hdr = _shl(buf[h, pl.ds(hrow, 1), :], -bit)
        tiles, flags = [_values(w[:64], hdr), _values(w[64:], _shl(hdr, -8))], hdr & 0x8080
        if live is not None:
            tiles, flags = [jnp.where(live, t, 0.0) for t in tiles], jnp.where(live, flags, 0)
        return tiles, flags

    inbox = [{(0, 0): []}, {(0, 0): []}]
    for i, (r0, nr, c0) in enumerate(RAMP):
        land(RAMP_NEEDS[i])
        z = mm((0, 1), c0, L, r0, nr).astype(BF)
        rs, cs = pl.ds(r0, nr), pl.ds(c0, L)
        for q, h in enumerate(H):
            s1[h, rs, cs] = z[q * nr:(q + 1) * nr]
        if i == 0:
            pl.semaphore_wait(barrier, 2)
        for q, h in enumerate(H):
            inbox[q][0, 0].append(send(s1.at[h, rs, cs], r1.at[h, rs, cs], h, h))
    for q, h in enumerate(H):
        land(7 + q)
        put_unit(ps1, h, AT1[1, 0], mm((2 + q,), 0, U))
        inbox[q][1, 0] = [send1(h, M10)]
    land(9)
    for s, msg in enumerate((M01, M11)):
        z = mm((2 * s, 2 * s + 1), U, U)
        for q, h in enumerate(H):
            put_unit(ps1, h, AT1[s, 1], z[q * RB:(q + 1) * RB])
            inbox[q][s, 1] = [send1(h, msg)]

    via2 = [me == 1 + 2 * h for h in H]

    def cp_a(h, msg):
        return remote(ps1.at[h, pl.ds(*msg)], pr1.at[h, pl.ds(*msg)], sem_x.at[h], sem_x.at[2 + h], h)

    def cp_x(h):
        return remote(ps1.at[h, pl.ds(*MX)], px.at[h, pl.ds(7, MX[1])], sem_x.at[4], sem_x.at[5 + h], 1 - h)

    land(10)
    z = mm((0, 1), 2 * U, 2 * U)
    for q, h in enumerate(H):
        for c in (3, 2):
            put_unit(ps1, h, AT1[0, c], z[q * RB:(q + 1) * RB, (c - 2) * U:(c - 1) * U])
    for q, h in enumerate(H):
        pl.when(via2[q])(lambda: cp_x(h).start())
    z = mm((2, 3), 2 * U, 2 * U)
    zb[...] = z[:, U:]
    for q, h in enumerate(H):
        put_unit(ps1, h, AT1[1, 2], z[q * RB:(q + 1) * RB, :U])
    for q, h in enumerate(H):
        pl.when(via2[q])(lambda: cp_a(h, MY).start())
        pl.when(jnp.logical_not(via2[q]))(lambda: cp_a(h, MA).start())
    land(12)
    acc[pl.ds(0, 2 * RB), :] = mm((4, 5), 0, N)

    @pl.when(is2)
    def _():
        for h in range(2):
            cp_x(h).wait_recv()

    for q, h in enumerate(H):
        p, flags = get_unit(px, h, (8, 7, 0), is2)
        put_unit(ps1, h, AT1[1, 3], zb[pl.ds(q * RB, RB), :] + jnp.concatenate(p, axis=1), flags)
        inbox[q][1, 3] = [send1(h, M13)]
    land(14)
    acc[pl.ds(2 * RB, 2 * RB), :] = mm((6, 7), 0, N)

    def partner(s, c, q):
        h = H[q]
        for cp in inbox[q].get((s, c), ()):
            cp.wait_recv()
        if (s, c) == (0, 0):
            return [r1[h, :, pl.ds(e * L, L)].astype(F32) for e in range(2)], 0
        if (s, c) == (0, 2):
            pl.when(is0)(lambda: cp_a(h, MY).wait_recv())
            pl.when(jnp.logical_not(is0))(lambda: cp_a(h, MA).wait_recv())
        return get_unit(pr1, h, AT1[s, c], jnp.logical_not(is0) if (s, c) == (0, 3) else None)

    rs2 = [[], []]
    for i, msg in enumerate(M2):
        for q, h in enumerate(H):
            for c in (2 * i, 2 * i + 1):
                p, flags = partner(0, c, q)
                put_unit(ps2, h, AT2[c], acc[pl.ds(q * RB, RB), pl.ds(c * U, U)] + jnp.concatenate(p, axis=1), flags)
            rs2[q].append(send(ps2.at[h, pl.ds(*msg)], pr2.at[h, pl.ds(*msg)], h, 1 - h))

    ag1 = [[], []]
    for i, msg in enumerate(AG_OWN):
        for q, h in enumerate(H):
            rs2[q][i].wait_recv()
            hdr = 0
            for c in (2 * i, 2 * i + 1):
                p1, f1 = partner(1, c, q)
                p2, f2 = get_unit(pr2, h, AT2[c])
                hdr = hdr | _shl(f1 | f2, 16 * (c % 2))
                for e in range(2):
                    j = 2 * c + e
                    z = acc[pl.ds((2 + q) * RB, RB), pl.ds(j * L, L)] + p1[e] + p2[e]
                    hd, w = _words(jnp.maximum(z, 0.0), False)
                    hdr = hdr | _shl(hd, 8 * (j % 4))
                    pg[h, pl.ds(G_ROW[j], 48), :] = _squeeze12(w)
            pg[h, pl.ds(G_HDR[4 * i], 1), :] = hdr
            ag1[q].append(send(pg.at[h, pl.ds(*msg)], pg.at[2 + h, pl.ds(*msg)], h, 1 - h))

    def emit(k, h, tiles):
        for j in tiles:
            o_ref[pl.ds(block_row(3 - k, h), RB), pl.ds(j * L, L)] = _values(
                _expand12(pg[2 * k + h, pl.ds(G_ROW[j], 48), :]),
                _shl(pg[2 * k + h, pl.ds(G_HDR[j], 1), :], -8 * (j % 4)))

    ag2 = [send(pg.at[h, pl.ds(0, PG)], pg.at[4 + h, pl.ds(0, PG)], h, h) for h in H]
    for h in H:
        emit(0, h, range(8))
    fwd = []
    for q, h in enumerate(H):
        for cp in ag1[q]:
            cp.wait_recv()
        fwd.append([remote(pg.at[2 + h, pl.ds(*msg)], pg.at[6 + h, pl.ds(*msg)], sem_s.at[2 * (N_MSG - 2 + e) + h],
                           sem_r.at[2 * (N_MSG - 2 + e) + h], h) for e, msg in enumerate(AG_FWD)])
        fwd[q][0].start()
        pl.when(jnp.logical_not(is2))(lambda: fwd[q][1].start())

    def cp_last(h):
        rows = pl.ds(*AG_FWD[1])
        return remote(pg.at[4 + h, rows], pg.at[6 + h, rows], sem_x.at[7 + h], sem_r.at[2 * (N_MSG - 1) + h], 1 - h)

    for h in H:
        emit(1, h, range(8))
    for q in (1, 0):
        ag2[q].wait_recv()
        pl.when(is0)(lambda: cp_last(H[q]).start())
        emit(2, H[q], range(8))
    for q in (1, 0):
        fwd[q][0].wait_recv()
        emit(3, H[q], range(NF))

    flags = 0
    for k in range(8):
        flags = flags | pg[k, pl.ds(G_HDR[0], 1), :] | pg[k, pl.ds(G_HDR[4], 1), :]
    miss = jnp.max(_shl(flags & _i32(0x80808080), -1)) > 0

    for cp in sent + [fwd[0][0], fwd[1][0]]:
        cp.wait_send()
    for q, h in enumerate(H):
        @pl.when(via2[q])
        def _():
            cp_x(h).wait_send()
            cp_a(h, MY).wait_send()

        pl.when(jnp.logical_not(via2[q]))(lambda: cp_a(h, MA).wait_send())
        pl.when(jnp.logical_not(is2))(lambda: fwd[q][1].wait_send())
        pl.when(is0)(lambda: cp_last(h).wait_send())

    @pl.when(miss)
    def _():
        for q in range(2):
            fwd[q][1].wait_recv()

        def rows(i, n=1):
            return pl.ds(pl.multiple_of(i * RB, RB), n * RB)

        def exchange(k, src, dst, first_link):
            cps = [remote(src(h), dst(h), sem_fs.at[h], sem_fr.at[2 * k + h], h if first_link else 1 - h)
                   for h in range(2)]
            for cp in cps:
                cp.start()
            for cp in cps:
                cp.wait()

        def for_units(n_blocks, f):
            @pl.loop(0, 4 * n_blocks)
            def _(t):
                f(t >> 2, pl.ds(pl.multiple_of((t & 3) * U, U), U))

        def partial(i, cs):
            lhs = a16[rows(2 * (i & 1) + ((i >> 1) ^ first)), :]
            fs1[rows(i), cs] = jnp.dot(lhs, b16[:, cs], preferred_element_type=F32).astype(BF)

        def pair_sum(h, cs):
            fs2[rows(h), cs] = (acc[rows(h ^ first), cs] + fr1[rows(2 * h), cs].astype(F32)).astype(BF)

        def finish(h, cs):
            z = acc[rows(2 + (h ^ first)), cs] + fr1[rows(2 * h + 1), cs].astype(F32) + fr2[rows(h), cs].astype(F32)
            fg[rows(4 * h), cs] = jnp.maximum(z, 0.0).astype(BF)

        def write(i, cs):
            h = i >> 2
            u = jnp.where(h == 0, y, x) ^ ((i >> 1) & 1)
            v = jnp.where(h == 0, x, y) ^ (i & 1)
            o_ref[rows(4 * h + 2 * u + v), cs] = fg[rows(i), cs].astype(F32)

        for_units(4, partial)
        exchange(0, lambda h: fs1.at[pl.ds(2 * h * RB, 2 * RB)], lambda h: fr1.at[pl.ds(2 * h * RB, 2 * RB)], True)
        for_units(2, pair_sum)
        exchange(1, lambda h: fs2.at[pl.ds(h * RB, RB)], lambda h: fr2.at[pl.ds(h * RB, RB)], False)
        for_units(2, finish)
        exchange(2, lambda h: fg.at[pl.ds(4 * h * RB, RB)], lambda h: fg.at[pl.ds((4 * h + 1) * RB, RB)], False)
        exchange(3, lambda h: fg.at[pl.ds(4 * h * RB, 2 * RB)], lambda h: fg.at[pl.ds((4 * h + 2) * RB, 2 * RB)], True)
        for_units(8, write)

    @pl.when(jnp.logical_not(miss))
    def _():
        for q in (1, 0):
            fwd[q][1].wait_recv()
            emit(3, H[q], range(NF, 8))


def pallas_dist_matmul_relu_kshard_i_m1024_n1024_k512_kernel(A: jax.Array, B: jax.Array):
    vmem, dma = pltpu.VMEM, pltpu.SemaphoreType.DMA
    return pl.pallas_call(
        _body,
        out_shape=jax.ShapeDtypeStruct((M, N), F32),
        in_specs=[pl.BlockSpec(memory_space=pltpu.HBM)] * 2,
        out_specs=pl.BlockSpec(memory_space=pltpu.VMEM),
        scratch_shapes=[
            vmem((M, KS), F32), vmem((KS, N), F32), vmem((M, KS), BF), vmem((KS, N), BF),
            vmem((4 * RB, N), F32),
            vmem((2, RB, U), BF), vmem((2, RB, U), BF),
            vmem((2, P1, L), I32), vmem((2, P1, L), I32),
            vmem((2, P2, L), I32), vmem((2, P2, L), I32),
            vmem((8, 392, L), I32),
            vmem((2 * RB, U), F32), vmem((2, 112, L), I32),
            vmem((4 * RB, N), BF), vmem((4 * RB, N), BF),
            vmem((2 * RB, N), BF), vmem((2 * RB, N), BF), vmem((8 * RB, N), BF),
            dma((len(LOADS),)), dma((2 * N_MSG,)), dma((2 * N_MSG,)), dma((9,)), dma((2,)), dma((8,)),
        ],
        compiler_params=pltpu.CompilerParams(collective_id=0, vmem_limit_bytes=48 * 1024 * 1024,
                                             disable_semaphore_checks=True),
    )(A, B)
```

```python
import jax
import jax.numpy as jnp
from jax import lax
from jax.experimental import pallas as pl
from jax.experimental.pallas import tpu as pltpu

M, N, KS = 1024, 1024, 512
RB = 128
L = 128
U = 256

BF, F32, I32 = jnp.bfloat16, jnp.float32, jnp.int32
SIGN = -(1 << 31)


def _i32(v):
    return v - (1 << 32) if v >= (1 << 31) else v


def _rep(v):
    return _i32(v | (v << 16))


def _shl(x, n):
    return x if n == 0 else (lax.shift_left(x, n) if n > 0 else lax.shift_right_logical(x, -n))


def _words(tile, signed):
    bits = pltpu.bitcast(tile, I32)
    mag = bits & 0x7FFFFFFF if signed else bits
    top = pltpu.bitcast(jnp.max(pltpu.bitcast(mag, F32), axis=0, keepdims=True), I32)
    low = pltpu.bitcast(jnp.max(pltpu.bitcast(SIGN - mag, F32), axis=0, keepdims=True), I32) & 0x7FFFFFFF
    base = jnp.maximum(lax.shift_right_logical(top + 0x8000, 23) - 31, 0)
    miss = (base > 126) | (low > SIGN - lax.shift_left(base + 1, 23))
    tile = tile * pltpu.bitcast(lax.shift_left(127 - base, 23), F32)
    return jnp.where(miss, 0x80, base), pltpu.bitcast(tile.astype(BF), I32)


def _values(w, hdr):
    return pltpu.bitcast(w, BF).astype(F32) * pltpu.bitcast(lax.shift_left((hdr & 0x7F) + 127, 23), F32)


def _squeeze12(w):
    return jnp.concatenate([w[16 * j:16 * j + 16] | (_shl(w[48:], 12 - 4 * j) & _rep(0xF000)) for j in range(3)],
                           axis=0)


def _expand12(r):
    e = [_shl(r[16 * j:16 * j + 16] & _rep(0xF000), 4 * j - 12) for j in range(3)]
    return jnp.concatenate([r & _rep(0x0FFF), e[0] | e[1] | e[2]], axis=0)


def _squeeze13(w):
    p = [w[8 * j:8 * j + 8] for j in range(16)]
    out = [p[j] | (_shl(p[13 + j // 4], 12 - 3 * (j % 4)) & _rep(0x7000)) for j in range(12)]
    s = [_shl(p[13 + j] & _rep(0x8000), -1 - j) for j in range(3)]
    return jnp.concatenate(out + [p[12] | s[0] | s[1] | s[2]], axis=0)


def _expand13(r):
    p = [r[8 * j:8 * j + 8] for j in range(13)]
    ext = []
    for e in range(3):
        v = _shl(p[12], 1 + e) & _rep(0x8000)
        for q in range(4):
            v = v | _shl(p[4 * e + q] & _rep(0x7000), 3 * q - 12)
        ext.append(v)
    return jnp.concatenate([r & _rep(0x8FFF)] + ext, axis=0)


RAMP = ((0, 64, 0), (64, 64, 0), (0, 128, L))
LOADS = (
    ("b", 0, L), ("a", 0, 0, 0, 64), ("a", 0, 1, 0, 64), ("a", 0, 0, 64, 64), ("a", 0, 1, 64, 64), ("b", L, L),
    ("a", 1, 0, 0, RB), ("a", 1, 1, 0, RB), ("b", U, U), ("b", 2 * U, 2 * U),
    ("a", 2, 0, 0, RB), ("a", 2, 1, 0, RB), ("a", 3, 0, 0, RB), ("a", 3, 1, 0, RB),
)
RAMP_NEEDS = (3, 5, 6)

AT1 = {(1, 0): (0, 104, 0), (0, 1): (112, 216, 0), (1, 1): (224, 223, 0),
       (0, 3): (336, 335, 0), (0, 2): (440, 648, 0), (1, 2): (544, 648, 16), (1, 3): (656, 655, 0)}
P1 = 760
M10, M01, M11, M13 = (0, 105), (112, 105), (223, 105), (655, 105)
MA, MX, MY = (335, 314), (335, 105), (440, 209)
AT2 = tuple((104 * c + 8 * (c // 2), 208 + 7 * (c // 2), 16 * (c % 2)) for c in range(4))
P2 = 424
M2 = ((0, 209), (215, 209))
G_ROW = tuple(48 * j + 2 * (j // 4) for j in range(8))
G_HDR = tuple(192 + j // 4 for j in range(8))
PG = 386
AG_OWN = ((0, 193), (193, 193))
NF = 6
AG_FWD = ((0, G_ROW[NF]), (G_ROW[NF], PG - G_ROW[NF]))
N_MSG = len(RAMP) + 4 + 2 + 2 + 1 + 2


def _body(a_hbm, b_hbm, o_ref, a32, b32, a16, b16, acc, s1, r1, ps1, pr1, ps2, pr2, pg, zb, px,
          fs1, fr1, fs2, fr2, fg, sem_in, sem_s, sem_r, sem_x, sem_fs, sem_fr):
    me = lax.axis_index("i")
    x = me >> 1
    y = (me & 1) ^ x
    first = jnp.where(me == 1, 1, 0)
    H = (first, 1 - first)
    is0, is2 = me == 0, me == 2

    def peer(link):
        return (me ^ (1 + 2 * link),)

    def block_row(s, h, r0=0):
        u = jnp.where(h == 0, y, x) ^ (1 - s // 2)
        v = jnp.where(h == 0, x, y) ^ (1 - s % 2)
        return pl.multiple_of((4 * h + 2 * u + v) * RB + r0, 16)

    loads = []
    for i, ld in enumerate(LOADS):
        if ld[0] == "a":
            _, s, q, r0, nr = ld
            cp = pltpu.make_async_copy(a_hbm.at[pl.ds(block_row(s, H[q], r0), nr)],
                                       a32.at[pl.ds((2 * s + q) * RB + r0, nr)], sem_in.at[i])
        else:
            cs = pl.ds(*ld[1:])
            cp = pltpu.make_async_copy(b_hbm.at[:, cs], b32.at[:, cs], sem_in.at[i])
        cp.start()
        loads.append(cp)
        if i == RAMP_NEEDS[0] - 1:
            barrier = pltpu.get_barrier_semaphore()
            for link in range(2):
                pl.semaphore_signal(barrier, inc=1, device_id=peer(link), device_id_type=pl.DeviceIdType.MESH)
    landed = [0]

    def land(n):
        for i in range(landed[0], n):
            loads[i].wait()
            if LOADS[i][0] == "a":
                _, s, q, r0, nr = LOADS[i]
                rs = pl.ds((2 * s + q) * RB + r0, nr)
                a16[rs, :] = a32[rs, :].astype(BF)
            else:
                cs = pl.ds(*LOADS[i][1:])
                b16[:, cs] = b32[:, cs].astype(BF)
        landed[0] = n

    def remote(src, dst, send_sem, recv_sem, link):
        return pltpu.make_async_remote_copy(src, dst, send_sem, recv_sem, device_id=peer(link),
                                            device_id_type=pl.DeviceIdType.MESH)

    sent = []

    def send(src, dst, h, link):
        k = len(sent) // 2 * 2 + h
        cp = remote(src, dst, sem_s.at[k], sem_r.at[k], link)
        cp.start()
        sent.append(cp)
        return cp

    def send1(h, msg):
        return send(ps1.at[h, pl.ds(*msg)], pr1.at[h, pl.ds(*msg)], h, h)

    def mm(blocks, c0, nc, r0=0, nr=RB):
        lhs = jnp.concatenate([a16[pl.ds(b * RB + r0, nr), :] for b in blocks], axis=0)
        return jnp.dot(lhs, b16[:, pl.ds(c0, nc)], preferred_element_type=F32)

    def put_unit(buf, h, at, vals, flags=0):
        row, hrow, bit = at
        (h0, w0), (h1, w1) = _words(vals[:, :L], True), _words(vals[:, L:], True)
        hdr = _shl(h0 | _shl(h1, 8) | flags, bit)
        buf[h, pl.ds(hrow, 1), :] = hdr | buf[h, pl.ds(hrow, 1), :] if bit else hdr
        buf[h, pl.ds(row, 104), :] = _squeeze13(jnp.concatenate([w0, w1], axis=0))

    def get_unit(buf, h, at, live=None):
        row, hrow, bit = at
        w = _expand13(buf[h, pl.ds(row, 104), :])
        hdr = _shl(buf[h, pl.ds(hrow, 1), :], -bit)
        tiles, flags = [_values(w[:64], hdr), _values(w[64:], _shl(hdr, -8))], hdr & 0x8080
        if live is not None:
            tiles, flags = [jnp.where(live, t, 0.0) for t in tiles], jnp.where(live, flags, 0)
        return tiles, flags

    inbox = [{(0, 0): []}, {(0, 0): []}]
    for i, (r0, nr, c0) in enumerate(RAMP):
        land(RAMP_NEEDS[i])
        z = mm((0, 1), c0, L, r0, nr).astype(BF)
        rs, cs = pl.ds(r0, nr), pl.ds(c0, L)
        for q, h in enumerate(H):
            s1[h, rs, cs] = z[q * nr:(q + 1) * nr]
        if i == 0:
            pl.semaphore_wait(barrier, 2)
        for q, h in enumerate(H):
            inbox[q][0, 0].append(send(s1.at[h, rs, cs], r1.at[h, rs, cs], h, h))
    for q, h in enumerate(H):
        land(7 + q)
        put_unit(ps1, h, AT1[1, 0], mm((2 + q,), 0, U))
        inbox[q][1, 0] = [send1(h, M10)]
    land(9)
    for s, msg in enumerate((M01, M11)):
        z = mm((2 * s, 2 * s + 1), U, U)
        for q, h in enumerate(H):
            put_unit(ps1, h, AT1[s, 1], z[q * RB:(q + 1) * RB])
            inbox[q][s, 1] = [send1(h, msg)]

    via2 = [me == 1 + 2 * h for h in H]

    def cp_a(h, msg):
        return remote(ps1.at[h, pl.ds(*msg)], pr1.at[h, pl.ds(*msg)], sem_x.at[h], sem_x.at[2 + h], h)

    def cp_x(h):
        return remote(ps1.at[h, pl.ds(*MX)], px.at[h, pl.ds(7, MX[1])], sem_x.at[4], sem_x.at[5 + h], 1 - h)

    land(10)
    z = mm((0, 1), 2 * U, 2 * U)
    for q, h in enumerate(H):
        for c in (3, 2):
            put_unit(ps1, h, AT1[0, c], z[q * RB:(q + 1) * RB, (c - 2) * U:(c - 1) * U])
    for q, h in enumerate(H):
        pl.when(via2[q])(lambda: cp_x(h).start())
    z = mm((2, 3), 2 * U, 2 * U)
    zb[...] = z[:, U:]
    for q, h in enumerate(H):
        put_unit(ps1, h, AT1[1, 2], z[q * RB:(q + 1) * RB, :U])
    for q, h in enumerate(H):
        pl.when(via2[q])(lambda: cp_a(h, MY).start())
        pl.when(jnp.logical_not(via2[q]))(lambda: cp_a(h, MA).start())
    land(12)
    acc[pl.ds(0, 2 * RB), :] = mm((4, 5), 0, N)

    @pl.when(is2)
    def _():
        for h in range(2):
            cp_x(h).wait_recv()

    for q, h in enumerate(H):
        p, flags = get_unit(px, h, (8, 7, 0), is2)
        put_unit(ps1, h, AT1[1, 3], zb[pl.ds(q * RB, RB), :] + jnp.concatenate(p, axis=1), flags)
        inbox[q][1, 3] = [send1(h, M13)]
    land(14)
    acc[pl.ds(2 * RB, 2 * RB), :] = mm((6, 7), 0, N)

    def partner(s, c, q):
        h = H[q]
        for cp in inbox[q].get((s, c), ()):
            cp.wait_recv()
        if (s, c) == (0, 0):
            return [r1[h, :, pl.ds(e * L, L)].astype(F32) for e in range(2)], 0
        if (s, c) == (0, 2):
            pl.when(is0)(lambda: cp_a(h, MY).wait_recv())
            pl.when(jnp.logical_not(is0))(lambda: cp_a(h, MA).wait_recv())
        return get_unit(pr1, h, AT1[s, c], jnp.logical_not(is0) if (s, c) == (0, 3) else None)

    rs2 = [[], []]
    for i, msg in enumerate(M2):
        for q, h in enumerate(H):
            for c in (2 * i, 2 * i + 1):
                p, flags = partner(0, c, q)
                put_unit(ps2, h, AT2[c], acc[pl.ds(q * RB, RB), pl.ds(c * U, U)] + jnp.concatenate(p, axis=1), flags)
            rs2[q].append(send(ps2.at[h, pl.ds(*msg)], pr2.at[h, pl.ds(*msg)], h, 1 - h))

    ag1 = [[], []]
    for i, msg in enumerate(AG_OWN):
        for q, h in enumerate(H):
            rs2[q][i].wait_recv()
            hdr = 0
            for c in (2 * i, 2 * i + 1):
                p1, f1 = partner(1, c, q)
                p2, f2 = get_unit(pr2, h, AT2[c])
                hdr = hdr | _shl(f1 | f2, 16 * (c % 2))
                for e in range(2):
                    j = 2 * c + e
                    z = acc[pl.ds((2 + q) * RB, RB), pl.ds(j * L, L)] + p1[e] + p2[e]
                    hd, w = _words(jnp.maximum(z, 0.0), False)
                    hdr = hdr | _shl(hd, 8 * (j % 4))
                    pg[h, pl.ds(G_ROW[j], 48), :] = _squeeze12(w)
            pg[h, pl.ds(G_HDR[4 * i], 1), :] = hdr
            ag1[q].append(send(pg.at[h, pl.ds(*msg)], pg.at[2 + h, pl.ds(*msg)], h, 1 - h))

    def emit(k, h, tiles):
        for j in tiles:
            o_ref[pl.ds(block_row(3 - k, h), RB), pl.ds(j * L, L)] = _values(
                _expand12(pg[2 * k + h, pl.ds(G_ROW[j], 48), :]),
                _shl(pg[2 * k + h, pl.ds(G_HDR[j], 1), :], -8 * (j % 4)))

    ag2 = [send(pg.at[h, pl.ds(0, PG)], pg.at[4 + h, pl.ds(0, PG)], h, h) for h in H]
    for h in H:
        emit(0, h, range(8))
    fwd = []
    for q, h in enumerate(H):
        for cp in ag1[q]:
            cp.wait_recv()
        fwd.append([remote(pg.at[2 + h, pl.ds(*msg)], pg.at[6 + h, pl.ds(*msg)], sem_s.at[2 * (N_MSG - 2 + e) + h],
                           sem_r.at[2 * (N_MSG - 2 + e) + h], h) for e, msg in enumerate(AG_FWD)])
        fwd[q][0].start()
        pl.when(jnp.logical_not(is2))(lambda: fwd[q][1].start())

    def cp_last(h):
        rows = pl.ds(*AG_FWD[1])
        return remote(pg.at[4 + h, rows], pg.at[6 + h, rows], sem_x.at[7 + h], sem_r.at[2 * (N_MSG - 1) + h], 1 - h)

    for h in H:
        emit(1, h, range(8))
    for q in (1, 0):
        ag2[q].wait_recv()
        pl.when(is0)(lambda: cp_last(H[q]).start())
        emit(2, H[q], range(8))
    for q in (1, 0):
        fwd[q][0].wait_recv()
        emit(3, H[q], range(NF))

    flags = 0
    for k in range(8):
        flags = flags | pg[k, pl.ds(G_HDR[0], 1), :] | pg[k, pl.ds(G_HDR[4], 1), :]
    miss = jnp.max(_shl(flags & _i32(0x80808080), -1)) > 0

    for cp in sent + [fwd[0][0], fwd[1][0]]:
        cp.wait_send()
    for q, h in enumerate(H):
        @pl.when(via2[q])
        def _():
            cp_x(h).wait_send()
            cp_a(h, MY).wait_send()

        pl.when(jnp.logical_not(via2[q]))(lambda: cp_a(h, MA).wait_send())
        pl.when(jnp.logical_not(is2))(lambda: fwd[q][1].wait_send())
        pl.when(is0)(lambda: cp_last(h).wait_send())

    @pl.when(miss)
    def _():
        for q in range(2):
            fwd[q][1].wait_recv()

        def rows(i, n=1):
            return pl.ds(pl.multiple_of(i * RB, RB), n * RB)

        def exchange(k, src, dst, first_link):
            cps = [remote(src(h), dst(h), sem_fs.at[h], sem_fr.at[2 * k + h], h if first_link else 1 - h)
                   for h in range(2)]
            for cp in cps:
                cp.start()
            for cp in cps:
                cp.wait()

        def for_units(n_blocks, f):
            @pl.loop(0, 4 * n_blocks)
            def _(t):
                f(t >> 2, pl.ds(pl.multiple_of((t & 3) * U, U), U))

        def partial(i, cs):
            lhs = a16[rows(2 * (i & 1) + ((i >> 1) ^ first)), :]
            fs1[rows(i), cs] = jnp.dot(lhs, b16[:, cs], preferred_element_type=F32).astype(BF)

        def pair_sum(h, cs):
            fs2[rows(h), cs] = (acc[rows(h ^ first), cs] + fr1[rows(2 * h), cs].astype(F32)).astype(BF)

        def finish(h, cs):
            z = acc[rows(2 + (h ^ first)), cs] + fr1[rows(2 * h + 1), cs].astype(F32) + fr2[rows(h), cs].astype(F32)
            fg[rows(4 * h), cs] = jnp.maximum(z, 0.0).astype(BF)

        def write(i, cs):
            h = i >> 2
            u = jnp.where(h == 0, y, x) ^ ((i >> 1) & 1)
            v = jnp.where(h == 0, x, y) ^ (i & 1)
            o_ref[rows(4 * h + 2 * u + v), cs] = fg[rows(i), cs].astype(F32)

        for_units(4, partial)
        exchange(0, lambda h: fs1.at[pl.ds(2 * h * RB, 2 * RB)], lambda h: fr1.at[pl.ds(2 * h * RB, 2 * RB)], True)
        for_units(2, pair_sum)
        exchange(1, lambda h: fs2.at[pl.ds(h * RB, RB)], lambda h: fr2.at[pl.ds(h * RB, RB)], False)
        for_units(2, finish)
        exchange(2, lambda h: fg.at[pl.ds(4 * h * RB, RB)], lambda h: fg.at[pl.ds((4 * h + 1) * RB, RB)], False)
        exchange(3, lambda h: fg.at[pl.ds(4 * h * RB, 2 * RB)], lambda h: fg.at[pl.ds((4 * h + 2) * RB, 2 * RB)], True)
        for_units(8, write)

    @pl.when(jnp.logical_not(miss))
    def _():
        for q in (1, 0):
            fwd[q][1].wait_recv()
            emit(3, H[q], range(NF, 8))


def pallas_dist_matmul_relu_kshard_i_m1024_n1024_k512_kernel(A: jax.Array, B: jax.Array):
    vmem, dma = pltpu.VMEM, pltpu.SemaphoreType.DMA
    return pl.pallas_call(
        _body,
        out_shape=jax.ShapeDtypeStruct((M, N), F32),
        in_specs=[pl.BlockSpec(memory_space=pltpu.HBM)] * 2,
        out_specs=pl.BlockSpec(memory_space=pltpu.VMEM),
        scratch_shapes=[
            vmem((M, KS), F32), vmem((KS, N), F32), vmem((M, KS), BF), vmem((KS, N), BF),
            vmem((4 * RB, N), F32),
            vmem((2, RB, U), BF), vmem((2, RB, U), BF),
            vmem((2, P1, L), I32), vmem((2, P1, L), I32),
            vmem((2, P2, L), I32), vmem((2, P2, L), I32),
            vmem((8, 392, L), I32),
            vmem((2 * RB, U), F32), vmem((2, 112, L), I32),
            vmem((4 * RB, N), BF), vmem((4 * RB, N), BF),
            vmem((2 * RB, N), BF), vmem((2 * RB, N), BF), vmem((8 * RB, N), BF),
            dma((len(LOADS),)), dma((2 * N_MSG,)), dma((2 * N_MSG,)), dma((9,)), dma((2,)), dma((8,)),
        ],
        compiler_params=pltpu.CompilerParams(collective_id=0, vmem_limit_bytes=48 * 1024 * 1024,
                                             disable_semaphore_checks=True),
    )(A, B)
```
